```python
import numpy as np

kernel_name = "dist_mean_ax0_shard0_i_m2048_n1024"

def setup_inputs():
    return {"x": np.random.randn(8192, 1024).astype(np.float32)}

def reference(x: np.ndarray) -> np.ndarray:
    return np.mean(x, axis=0, keepdims=True)
```

```python
import jax
import jax.numpy as jnp
from jax import lax
from jax.experimental import pallas as pl
from jax.experimental.pallas import tpu as pltpu

N_DEV = 4
N_CHUNKS = 8


def pallas_dist_mean_ax0_shard0_i_m2048_n1024_kernel(
x: jax.Array,
):
    m, n = x.shape
    rows = m // N_CHUNKS
    scale = 1.0 / (m * N_DEV)

    def kernel_body(x_hbm, out_ref, buf, parts, load_sems, send_sems, recv_sems):
        me = lax.axis_index("i")
        loads = [
            pltpu.make_async_copy(
                x_hbm.at[pl.ds(c * rows, rows)], buf.at[c], load_sems.at[c]
            )
            for c in range(N_CHUNKS)
        ]
        for ld in loads:
            ld.start()

        barrier = pltpu.get_barrier_semaphore()
        for d in range(1, N_DEV):
            pl.semaphore_signal(
                barrier, inc=1, device_id=((me + d) % N_DEV,),
                device_id_type=pl.DeviceIdType.MESH,
            )

        acc = jnp.zeros((8, n), jnp.float32)
        for c in range(N_CHUNKS):
            loads[c].wait()
            acc = acc + jnp.sum(buf[c].reshape(rows // 8, 8, n), axis=0)
        parts[0] = jnp.sum(acc, axis=0, keepdims=True)

        pl.semaphore_wait(barrier, N_DEV - 1)
        sends = []
        for d in range(1, N_DEV):
            rdma = pltpu.make_async_remote_copy(
                src_ref=parts.at[0], dst_ref=parts.at[d],
                send_sem=send_sems.at[d - 1], recv_sem=recv_sems.at[d - 1],
                device_id=((me + d) % N_DEV,),
                device_id_type=pl.DeviceIdType.MESH,
            )
            rdma.start()
            sends.append(rdma)
        for rdma in sends:
            rdma.wait_recv()
        out_ref[...] = ((parts[0] + parts[2]) + (parts[1] + parts[3])) * scale
        for rdma in sends:
            rdma.wait_send()

    return pl.pallas_call(
        kernel_body,
        out_shape=jax.ShapeDtypeStruct((1, n), x.dtype),
        in_specs=[pl.BlockSpec(memory_space=pl.ANY)],
        out_specs=pl.BlockSpec(memory_space=pltpu.VMEM),
        scratch_shapes=[
            pltpu.VMEM((N_CHUNKS, rows, n), jnp.float32),
            pltpu.VMEM((N_DEV, 1, n), jnp.float32),
            pltpu.SemaphoreType.DMA((N_CHUNKS,)),
            pltpu.SemaphoreType.DMA((N_DEV - 1,)),
            pltpu.SemaphoreType.DMA((N_DEV - 1,)),
        ],
        compiler_params=pltpu.CompilerParams(collective_id=0),
    )(x)
```

```python
import jax
import jax.numpy as jnp
from jax import lax
from jax.experimental import pallas as pl
from jax.experimental.pallas import tpu as pltpu

N_DEV = 4
SUBLANES = 8
NARROW = 128

FULL_CHUNKS = (1536, 288)
WIDE_CHUNKS = (184, 40)
NARROW_CHUNKS = (208, 16)
LOOP_ROWS = 32

FAR = 2
NEAR = (1, 3)


def _spans(chunks):
    return [(sum(chunks[:c]), rows) for c, rows in enumerate(chunks)]


def _tree_sum(values):
    while len(values) > 1:
        pairs = [a + b for a, b in zip(values[0::2], values[1::2])]
        values = pairs + values[2 * len(pairs):]
    return values[0]


def _fold_rows(ref, start, rows):
    block = ref[pl.ds(start, rows), :]
    return jnp.sum(block.reshape(rows // SUBLANES, SUBLANES, ref.shape[1]), axis=0)


def pallas_dist_mean_ax0_shard0_i_m2048_n1024_kernel(
x: jax.Array,
):
    m, n = x.shape
    full_rows = sum(FULL_CHUNKS)
    tail_rows = sum(WIDE_CHUNKS)
    wide = n - NARROW
    assert full_rows + tail_rows == m and sum(NARROW_CHUNKS) == tail_rows
    assert all(rows % LOOP_ROWS == 0 for rows in FULL_CHUNKS)
    scale = 1.0 / (m * N_DEV)

    def reduce_and_exchange(
        x_hbm, out_ref, full_buf, wide_buf, narrow_buf, parts,
        load_sems, send_sems, recv_sems,
    ):
        def start_loads(chunks, row0, cols, buf, sem0):
            loads = [
                pltpu.make_async_copy(
                    x_hbm.at[pl.ds(row0 + start, rows), cols],
                    buf.at[pl.ds(start, rows)],
                    load_sems.at[sem0 + c],
                )
                for c, (start, rows) in enumerate(_spans(chunks))
            ]
            for load in loads:
                load.start()
            return list(zip(loads, _spans(chunks)))

        all_cols, wide_cols, narrow_cols = (
            pl.ds(0, n), pl.ds(0, wide), pl.ds(wide, NARROW)
        )
        full_loads = start_loads(FULL_CHUNKS, 0, all_cols, full_buf, 0)
        wide_loads = start_loads(
            WIDE_CHUNKS, full_rows, wide_cols, wide_buf, len(FULL_CHUNKS)
        )
        narrow_loads = start_loads(
            NARROW_CHUNKS, full_rows, narrow_cols, narrow_buf,
            len(FULL_CHUNKS + WIDE_CHUNKS),
        )

        me = lax.axis_index("i")
        peer = {d: (me + d) % N_DEV for d in range(1, N_DEV)}

        barrier = pltpu.get_barrier_semaphore()
        for d in peer:
            pl.semaphore_signal(
                barrier, inc=1, device_id=(peer[d],),
                device_id_type=pl.DeviceIdType.MESH,
            )

        def send(slot, d, cols):
            copy = pltpu.make_async_remote_copy(
                src_ref=parts.at[0, :, cols],
                dst_ref=parts.at[d, :, cols],
                send_sem=send_sems.at[slot],
                recv_sem=recv_sems.at[slot],
                device_id=(peer[d],),
                device_id_type=pl.DeviceIdType.MESH,
            )
            copy.start()
            return copy

        acc = jnp.zeros((SUBLANES, n), jnp.float32)
        for load, (start, rows) in full_loads:
            load.wait()

            def step(j, acc, start=start):
                row = pl.multiple_of(start + j * LOOP_ROWS, SUBLANES)
                return acc + _fold_rows(full_buf, row, LOOP_ROWS)

            acc = lax.fori_loop(0, rows // LOOP_ROWS, step, acc)

        pl.semaphore_wait(barrier, N_DEV - 1)

        wide_acc = acc[:, :wide]
        for load, (start, rows) in wide_loads:
            load.wait()
            wide_acc = wide_acc + _fold_rows(wide_buf, start, rows)
        parts[0, :, wide_cols] = jnp.sum(wide_acc, axis=0, keepdims=True) * scale
        far_wide = send(0, FAR, wide_cols)

        narrow_acc = acc[:, wide:]
        for load, (start, rows) in narrow_loads:
            load.wait()
            tiles = [
                narrow_buf[pl.ds(row, SUBLANES), :]
                for row in range(start, start + rows, SUBLANES)
            ]
            narrow_acc = _tree_sum(tiles + [narrow_acc])
        parts[0, :, narrow_cols] = jnp.sum(narrow_acc, axis=0, keepdims=True) * scale
        far_narrow = send(1, FAR, narrow_cols)
        near = [send(2 + k, d, all_cols) for k, d in enumerate(NEAR)]

        for copy in (far_wide, far_narrow, *near):
            copy.wait_send()
        for copy in near:
            copy.wait_recv()
        own = parts[0]
        neighbours = parts[NEAR[0]] + parts[NEAR[1]]
        far_wide.wait_recv()
        far_narrow.wait_recv()
        out_ref[...] = ((own + parts[FAR]) + neighbours).astype(out_ref.dtype)

    def kernel_body(*refs):
        n_loads = len(FULL_CHUNKS + WIDE_CHUNKS + NARROW_CHUNKS)
        n_sends = 2 + len(NEAR)
        pl.run_scoped(
            lambda *sems: reduce_and_exchange(*refs, *sems),
            pltpu.SemaphoreType.DMA((n_loads,)),
            pltpu.SemaphoreType.DMA((n_sends,)),
            pltpu.SemaphoreType.DMA((n_sends,)),
        )

    return pl.pallas_call(
        kernel_body,
        out_shape=jax.ShapeDtypeStruct((1, n), x.dtype),
        in_specs=[pl.BlockSpec(memory_space=pltpu.HBM)],
        out_specs=pl.BlockSpec(memory_space=pltpu.VMEM),
        scratch_shapes=[
            pltpu.VMEM((full_rows, n), x.dtype),
            pltpu.VMEM((tail_rows, wide), x.dtype),
            pltpu.VMEM((tail_rows, NARROW), x.dtype),
            pltpu.VMEM((N_DEV, 1, n), jnp.float32),
        ],
        compiler_params=pltpu.CompilerParams(collective_id=0),
    )(x)
```
